```python
import numpy as np

kernel_name = "dist_embed_lookup_i_n2048_v16384_d1024"

def setup_inputs():
    table = np.random.randn(65536, 1024).astype(np.float32)
    idx = np.random.randint(0, 65536, size=(2048,)).astype(np.int32)
    return {"table": table, "idx": idx}

def reference(table: np.ndarray, idx: np.ndarray) -> np.ndarray:
    return table[idx]
```

```python
import jax
import jax.numpy as jnp
from jax import lax
from jax.experimental import pallas as pl
from jax.experimental.pallas import tpu as pltpu

N_DEV = 4
LANES = 128
HEAD = (16, 48, 64)
MESH = pl.DeviceIdType.MESH


def make(head=HEAD, handshake="chain", interpret=False, nobc=True):
    def kernel(table, idx):
        v_loc, d = table.shape
        n = idx.shape[0]
        shift = v_loc.bit_length() - 1
        n_rows = n // LANES
        wpr = d // (2 * LANES)
        n_head = len(head)
        starts = [sum(head[:k]) for k in range(n_head)]
        n_blk = n_head + n_rows - 1

        def body(table_ref, idx_ref, out_ref,
                 idx_s, own_s, meta_s, idx_v, meta_v, rows_v, comm_v, tmp_v,
                 misc_sem, gather_sem, send_sem, recv_sem, ready_sem):
            me = lax.axis_index("i")
            right = (me + 1) & 3
            left = (me + 3) & 3
            far = (me + 2) & 3
            peer = (right, left)

            def signal(sem, to):
                pl.semaphore_signal(sem, 1, device_id=(to,), device_id_type=MESH)

            head_cp = pltpu.make_async_copy(idx_ref.at[pl.ds(0, 1)], idx_s.at[pl.ds(0, 1)], misc_sem.at[0])
            rest_cp = pltpu.make_async_copy(idx_ref.at[pl.ds(1, n_rows - 1)], idx_s.at[pl.ds(1, n_rows - 1)], misc_sem.at[1])
            vec_cp = pltpu.make_async_copy(idx_ref, idx_v, misc_sem.at[2])
            meta_cp = pltpu.make_async_copy(meta_v, meta_s, misc_sem.at[3])
            head_cp.start()

            barrier = pltpu.get_barrier_semaphore()
            odd = (me & 1) == 1
            if handshake == "chain":
                @pl.when(me == 0)
                def _():
                    signal(barrier, 1)
                    signal(barrier, 3)

                @pl.when(odd)
                def _():
                    signal(barrier, 2)
            else:
                signal(barrier, left)
                signal(barrier, right)
            vec_cp.start()
            rest_cp.start()
            if handshake == "chain":
                @pl.when(odd)
                def _():
                    pl.semaphore_wait(barrier, 1)
                    signal(ready_sem, 0)

                @pl.when(me == 2)
                def _():
                    pl.semaphore_wait(barrier, 2)
                    signal(ready_sem, 1)
                    signal(ready_sem, 3)

            def row_copy(v, slot, blk):
                return pltpu.make_async_copy(
                    table_ref.at[pl.ds(v & (v_loc - 1), 1)], rows_v.at[slot], gather_sem.at[blk])

            def fetch(row, lane0, size, blk):
                base = row * LANES + lane0
                c = jnp.int32(0)
                for i in range(size):
                    v = idx_s[row, lane0 + i]
                    own_s[c] = v
                    c = c + (((v >> shift) & 3) == me).astype(jnp.int32)

                def issue(k, _):
                    row_copy(own_s[k], base + k, blk).start()
                lax.fori_loop(0, c, issue, None)
                return c

            def rounded(x):
                return pltpu.bitcast(x.astype(jnp.bfloat16).astype(jnp.float32), jnp.uint32)

            def pack(base, c, blk):
                @pl.when(c > 0)
                def _():
                    got = rows_v.at[pl.ds(base, c)]
                    pltpu.make_async_copy(got, got, gather_sem.at[blk]).wait()

                def group(g, _):
                    a = pl.multiple_of(base + 8 * g, 8)
                    x = rows_v[pl.ds(a, 8)].reshape(16 * wpr, LANES).astype(jnp.bfloat16)
                    comm_v[pl.ds(pl.multiple_of((me * n + a) * wpr, 8 * wpr), 8 * wpr), :] = pltpu.bitcast(x, jnp.uint32)
                lax.fori_loop(0, (c + 7) >> 3, group, None)

            def hop(slot, c, blk, kind, way):
                part = comm_v.at[pl.ds(slot * wpr, c * wpr)]
                return pltpu.make_async_remote_copy(
                    part, part, send_sem.at[way], recv_sem.at[4 * blk + 2 * kind + way],
                    device_id=(jnp.where(way == 0, right, left),), device_id_type=MESH)

            def send(base, c, blk, way):
                @pl.when(c > 0)
                def _():
                    hop(me * n + base, c, blk, 0, way).start()

            first = jnp.where(me == 1, 1, 0)
            head_cp.wait()
            cnt = [fetch(0, starts[0], head[0], 0)]
            for k in range(n_head):
                if k + 1 < n_head:
                    cnt.append(fetch(0, starts[k + 1], head[k + 1], k + 1))
                else:
                    rest_cp.wait()
                    c_next = fetch(1, 0, LANES, n_head)
                pack(starts[k], cnt[k], k)
                if k == 0:
                    if handshake == "chain":
                        @pl.when(me == 0)
                        def _():
                            pl.semaphore_wait(ready_sem, 2)
                    else:
                        pl.semaphore_wait(barrier, 2)
                send(starts[k], cnt[k], k, first)
            if handshake == "chain":
                @pl.when(odd)
                def _():
                    pl.semaphore_wait(ready_sem, 1)
            for k in range(n_head):
                send(starts[k], cnt[k], k, 1 - first)

            vec_cp.wait()
            owner = (idx_v[...] >> shift) & 3
            onehot = jnp.concatenate(
                [jnp.where(owner == o, 1.0, 0.0) for o in range(N_DEV)], axis=0).astype(jnp.bfloat16)
            q = lax.broadcasted_iota(jnp.int32, (LANES, LANES), 0)
            p = lax.broadcasted_iota(jnp.int32, (LANES, LANES), 1)

            def seg_start(x):
                s = jnp.zeros_like(x)
                for b in starts[1:]:
                    s = jnp.where(x >= b, b, s)
                return s

            def seg_id(x):
                s = jnp.zeros_like(x)
                for k, b in enumerate(starts):
                    s = jnp.where(x >= b, k, s)
                return s

            def count(mask):
                w = jnp.where(mask, 1.0, 0.0).astype(jnp.bfloat16)
                return jnp.dot(onehot, w, preferred_element_type=jnp.float32).astype(jnp.int32)

            def mine(x):
                r = x[0:n_rows]
                for o in range(1, N_DEV):
                    r = jnp.where(owner == o, x[o * n_rows:(o + 1) * n_rows], r)
                return r

            row = lax.broadcasted_iota(jnp.int32, (n_rows, LANES), 0)
            lane = lax.broadcasted_iota(jnp.int32, (n_rows, LANES), 1)
            rank = jnp.where(row == 0,
                             mine(count((q < p) & (q >= seg_start(p)))) + seg_start(lane),
                             mine(count(q < p)) + row * LANES)
            meta_v[0:n_rows, :] = (owner * n + rank) * wpr
            meta_v[n_rows:, :] = count((seg_id(q) == p) | (p >= n_head))
            meta_cp.start()

            def own_step(r, c):
                c_next = fetch(r + 1, 0, LANES, n_head + r)
                pack(r * LANES, c, n_head + r - 1)
                for way in range(2):
                    send(r * LANES, c, n_head + r - 1, way)
                return c_next
            c_last = lax.fori_loop(1, n_rows - 1, own_step, c_next)
            pack((n_rows - 1) * LANES, c_last, n_blk - 1)
            for way in range(2):
                send((n_rows - 1) * LANES, c_last, n_blk - 1, way)
            meta_cp.wait()

            def rows_of(o, r, k):
                return meta_s[n_rows + o * n_rows + r, k]

            def total(o):
                return lax.fori_loop(0, n_rows, lambda r, t: t + rows_of(o, r, n_head), jnp.int32(0), unroll=True)

            t_me, t_right, t_far, t_left = total(me), total(right), total(far), total(left)

            def rightward(bias, seen):
                return jnp.clip((bias + seen) >> 1, 0, seen)

            def in_relay_order(step, carry):
                carry = lax.fori_loop(
                    1, n_rows, lambda r, c: step(r, 0, LANES, n_head, n_head + r - 1, c), carry)
                for k in reversed(range(n_head)):
                    carry = step(0, starts[k], head[k], k, k, carry)
                return carry

            def relay(r, lane0, size, k, blk, seen):
                base = r * LANES + lane0
                new = []
                for way, (src, bias) in enumerate(((left, t_far - t_me), (right, t_me - t_far))):
                    c = rows_of(src, r, k)
                    cut = rightward(bias, seen[way] + c) - rightward(bias, seen[way])

                    @pl.when(c > 0)
                    def _():
                        hop(src * n + base, c, blk, 0, way).wait_recv()
                    lo, m = (0, cut) if way == 0 else (cut, c - cut)

                    @pl.when(m > 0)
                    def _():
                        hop(src * n + base + lo, m, blk, 1, way).start()
                    new.append(seen[way] + c)
                return tuple(new)
            in_relay_order(relay, (jnp.int32(0), jnp.int32(0)))

            def place(r, lane0, size, k, blk, seen):
                base = r * LANES + lane0
                c = rows_of(far, r, k)
                bias = t_right - t_left
                cut = rightward(bias, seen + c) - rightward(bias, seen)
                for way, (lo, m) in enumerate(((0, cut), (cut, c - cut))):
                    @pl.when(m > 0)
                    def _():
                        hop(far * n + base + lo, m, blk, 1, way).wait_recv()
                for i in range(size):
                    tmp_v[pl.ds(i * wpr, wpr), :] = comm_v[pl.ds(meta_s[r, lane0 + i], wpr), :]
                for g in range(size // 16):
                    at = pl.ds(pl.multiple_of(base + 16 * g, 16), 16)
                    for j in range(wpr):
                        ev = tmp_v[pl.ds(16 * g * wpr + j, 8, stride=2 * wpr), :]
                        od = tmp_v[pl.ds((16 * g + 1) * wpr + j, 8, stride=2 * wpr), :]
                        lo = (ev & 0xFFFF) | (od << 16)
                        hi = (ev >> 16) | (od & jnp.uint32(0xFFFF0000))
                        out_ref[at, pl.ds(2 * j * LANES, LANES)] = pltpu.bitcast(lo, jnp.bfloat16)
                        out_ref[at, pl.ds((2 * j + 1) * LANES, LANES)] = pltpu.bitcast(hi, jnp.bfloat16)
                return seen + c
            in_relay_order(place, jnp.int32(0))

            sent = (t_me + rightward(t_far - t_me, t_left),
                    t_me + t_right - rightward(t_me - t_far, t_right))
            for way in range(2):
                @pl.when(sent[way] > 0)
                def _():
                    hop(0, sent[way], 0, 0, way).wait_send()

        return pl.pallas_call(
            body,
            out_shape=jax.ShapeDtypeStruct((n, d), jnp.bfloat16),
            in_specs=[pl.BlockSpec(memory_space=pl.ANY), pl.BlockSpec(memory_space=pl.ANY)],
            out_specs=pl.BlockSpec(memory_space=pltpu.VMEM),
            scratch_shapes=[
                pltpu.SMEM((n_rows, LANES), jnp.int32),
                pltpu.SMEM((LANES + 1,), jnp.int32),
                pltpu.SMEM(((N_DEV + 1) * n_rows, LANES), jnp.int32),
                pltpu.VMEM((n_rows, LANES), jnp.int32),
                pltpu.VMEM(((N_DEV + 1) * n_rows, LANES), jnp.int32),
                pltpu.VMEM((n, 1, d), jnp.float32),
                pltpu.VMEM((N_DEV * n * wpr, LANES), jnp.uint32),
                pltpu.VMEM((LANES * wpr, LANES), jnp.uint32),
                pltpu.SemaphoreType.DMA((4,)),
                pltpu.SemaphoreType.DMA((n_blk,)),
                pltpu.SemaphoreType.DMA((2,)),
                pltpu.SemaphoreType.DMA((4 * n_blk,)),
                pltpu.SemaphoreType.REGULAR,
            ],
            compiler_params=pltpu.CompilerParams(
                collective_id=0, vmem_limit_bytes=64 << 20, disable_bounds_checks=nobc),
            interpret=interpret,
        )(table, idx.reshape(n_rows, LANES))
    return kernel


def pallas_dist_embed_lookup_i_n2048_v16384_d1024_kernel(table, idx):
    return make()(table, idx)
```

```python
import contextlib

import jax
import jax.numpy as jnp
from jax import lax
from jax.experimental import pallas as pl
from jax.experimental.pallas import tpu as pltpu

N_DEV = 4
LANES = 128
GROUP = 8
MESH = pl.DeviceIdType.MESH


def make(plan="f16/4 w v f28/6 f56/5V s f0/8 s f20/6 s g s n S s z n", tail=(64, 96, 112), early=5,
         interpret=False, checks=False, scopes=False, flags=None):
    scope = jax.named_scope if scopes else (lambda name: contextlib.nullcontext())

    def kernel(table, idx):
        v_loc, d = table.shape
        n = idx.shape[0]
        shift = v_loc.bit_length() - 1
        n_blk = n // LANES
        wpr = d // (2 * LANES)
        steps = plan.split()
        n_piece = sum(t[0] == "f" for t in steps)
        n_seg = n_blk + len(tail)

        def body(table_ref, idx_ref, out_ref,
                 head_s, pick_s, list_s, count_s, source_s,
                 idx_v, list_v, count_v, source_v, tall_v, rows_v, comm_v, tmp_v,
                 misc_sem, fetch_sem, send_sem, own_sem, far_sem, ready_sem):
            head_cp = pltpu.make_async_copy(idx_ref.at[pl.ds(0, 1)], head_s, misc_sem.at[0])
            vec_cp = pltpu.make_async_copy(idx_ref, idx_v, misc_sem.at[1])
            head_cp.start()
            vec_cp.start()

            me = lax.axis_index("i")
            right, far, left = (me + 1) & 3, (me + 2) & 3, (me + 3) & 3
            odd = (me & 1) == 1

            def signal(sem, to):
                pl.semaphore_signal(sem, 1, device_id=(to,), device_id_type=MESH)

            barrier = pltpu.get_barrier_semaphore()

            @pl.when(odd)
            def _():
                signal(barrier, 2)
                pl.semaphore_wait(barrier, 1)
                signal(ready_sem, 0)

            @pl.when(me == 0)
            def _():
                signal(barrier, 1)
                signal(barrier, 3)

            @pl.when(me == 2)
            def _():
                pl.semaphore_wait(barrier, 2)
                signal(ready_sem, 1)
                signal(ready_sem, 3)

            q = lax.broadcasted_iota(jnp.int32, (LANES, LANES), 0)
            p = lax.broadcasted_iota(jnp.int32, (LANES, LANES), 1)

            def running_count(flag):
                ones = jnp.where(flag, 1.0, 0.0).astype(jnp.bfloat16)
                through = jnp.where(q <= p, 1.0, 0.0).astype(jnp.bfloat16)
                return jnp.dot(ones, through, preferred_element_type=jnp.float32).astype(jnp.int32)

            def fetch_list(x, flag, count, blocks):
                half = (shift + 1) // 2
                low = x & (v_loc - 1)
                digits = jnp.concatenate([low >> half, low & ((1 << half) - 1)], axis=0)
                digits = digits.astype(jnp.float32).astype(jnp.bfloat16)
                goal = jnp.where(flag, count - 1, -1)
                blk = lax.broadcasted_iota(jnp.int32, x.shape, 0)
                front = jnp.zeros_like(x)
                for b in blocks:
                    route = jnp.where(goal[b:b + 1] == q, 1.0, 0.0).astype(jnp.bfloat16)
                    got = lax.dot_general(digits, route, (((1,), (1,)), ((), ())),
                                          preferred_element_type=jnp.float32).astype(jnp.int32)
                    front = jnp.where(blk == b, (got[:x.shape[0]] << half) | got[x.shape[0]:], front)
                return (front | (count << shift)).reshape(1, x.shape[0] * LANES)

            def fetch_row(entry, at, sem):
                pltpu.make_async_copy(
                    table_ref.at[pl.ds(entry & (v_loc - 1), 1)], rows_v.at[at], sem).start()

            def fetch(b, skip=0):
                c = (list_s[0, b * LANES + LANES - 1] >> shift) - skip
                last = b * LANES + jnp.minimum(c & -GROUP, LANES - GROUP)
                rows_v[pl.ds(last, GROUP)] = jnp.zeros((GROUP, 1, d), jnp.float32)
                lax.fori_loop(b * LANES, b * LANES + c,
                              lambda k, _: fetch_row(list_s[0, k + skip], k, fetch_sem.at[b]), None)
                return c

            def pack(base, c, sem, slot, single=False):
                @pl.when(c > 0)
                def _():
                    got = rows_v.at[pl.ds(base, c)]
                    pltpu.make_async_copy(got, got, sem).wait()

                def group(g, _):
                    x = rows_v[pl.ds(base + GROUP * g, GROUP)].reshape(2 * GROUP * wpr, LANES)
                    comm_v[pl.ds((slot + GROUP * g) * wpr, GROUP * wpr), :] = pltpu.bitcast(
                        x.astype(jnp.bfloat16), jnp.uint32)
                if single:
                    group(0, None)
                else:
                    lax.fori_loop(0, (c + GROUP - 1) >> 3, group, None)

            def hop(slot, c, recv_sems, k, way):
                part = comm_v.at[pl.ds(slot * wpr, c * wpr)]
                return pltpu.make_async_remote_copy(
                    part, part, send_sem.at[way], recv_sems.at[2 * k + way],
                    device_id=((me + 1 + 2 * way) & 3,), device_id_type=MESH)

            def send(slot, c, b, way):
                @pl.when(c > 0)
                def _():
                    hop(slot, c, own_sem, b, way).start()

            def ship(b, c):
                slot = me * n + b * LANES
                pack(b * LANES, c, fetch_sem.at[b], slot)
                with scope("s"):
                    for way in range(2):
                        send(slot, c, b, way)

            quick = pl.ds(0, early * LANES)
            quick_cp = pltpu.make_async_copy(list_v.at[:, quick], list_s.at[:, quick], misc_sem.at[2])
            first = jnp.where(me == 1, 1, 0)
            rows_v[pl.ds(n, GROUP * n_piece)] = jnp.zeros((GROUP * n_piece, 1, d), jnp.float32)
            with scope("idx"):
                head_cp.wait()
            pos, pieces, done, both, blk = 0, [], 0, False, 0
            others, fetched, packed = jnp.int32(0), jnp.int32(0), jnp.int32(0)
            for t in steps:
                if t[0] == "f":
                    size, room = map(int, t[1:].rstrip("V").split("/"))
                    base, sem = n + GROUP * len(pieces), fetch_sem.at[n_blk + len(pieces)]
                    for i in range(pos, pos + size):
                        v = head_s[0, i] ^ (me << shift)
                        pick_s[i - others] = v
                        other = jnp.minimum((v & ((N_DEV - 1) << shift)).astype(jnp.uint32), jnp.uint32(1))
                        others = others + other.astype(jnp.int32)
                    pos += size
                    c = jnp.minimum(pos - others - fetched, room)
                    if t[-1] == "V":
                        list_v[:, 0:8 * LANES] = fetch_list(x[0:8], flag[0:8], count[0:8], range(early))
                        quick_cp.start()

                    @pl.when(c > 0)
                    def _():
                        for k in range(room):
                            @pl.when(k < c)
                            def _():
                                fetch_row(pick_s[fetched + k], base + k, sem)
                    pieces.append((base, sem, c, True))
                    fetched = fetched + c
                elif t == "w":
                    vec_cp.wait()
                elif t == "v":
                    x = idx_v[...]
                    flag = ((x >> shift) & (N_DEV - 1)) == me
                    count = running_count(flag)
                elif t == "g":
                    with scope("g"):
                        quick_cp.wait()
                        pieces.append((0, fetch_sem.at[0], fetch(0, fetched), False))
                elif t == "n":
                    blk += 1
                    with scope("n"):
                        c_next = fetch(blk)
                elif t == "z":
                    ship(blk, c_next)
                else:
                    base, sem, c, single = pieces[done]
                    slot = me * n + packed
                    pack(base, c, sem, slot, single)
                    if done == 0:
                        @pl.when(me == 0)
                        def _():
                            pl.semaphore_wait(ready_sem, 2)
                    with scope("s"):
                        send(slot, c, 0, first)
                    if t == "S":
                        @pl.when(odd)
                        def _():
                            pl.semaphore_wait(ready_sem, 1)
                        held = jnp.where(odd, packed, 0)
                        send(slot - held, c + held, 0, 1 - first)
                        both = True
                    else:
                        send(slot, c if both else jnp.where(odd, 0, c), 0, 1 - first)
                    packed = packed + c
                    done += 1
            assert both and done == len(pieces)

            def stream(lo, hi, c):
                def step(b, c):
                    c_next = lax.cond(b + 1 < hi, lambda: fetch(b + 1), lambda: jnp.int32(0))
                    ship(b, c)
                    return c_next
                lax.fori_loop(lo, hi, step, c)
            stream(blk, early, c_next)

            rest = pl.ds(early * LANES, n - early * LANES)
            rest_cp = pltpu.make_async_copy(list_v.at[:, rest], list_s.at[:, rest], misc_sem.at[0])
            plan_cps = [pltpu.make_async_copy(count_v, count_s, misc_sem.at[1]),
                        pltpu.make_async_copy(source_v, source_s, misc_sem.at[2])]
            with scope("survey"):
                x = idx_v[...] & (N_DEV * v_loc - 1)
                blk = lax.broadcasted_iota(jnp.int32, (n_blk, LANES), 0)
                here = origin = blk * LANES + lax.broadcasted_iota(jnp.int32, (n_blk, LANES), 1)
                for b in range(n_blk):
                    tall_v[pl.ds(b * LANES, LANES), :] = jnp.broadcast_to(x[b:b + 1], (LANES, LANES)).T
                sub = lax.broadcasted_iota(jnp.int32, (8, LANES), 0)
                for end in range(n_blk, early, -4):
                    blocks = range(max(end - 4, early), end)
                    wide = [jnp.broadcast_to(x[b:b + 1], (8, LANES)) for b in blocks]

                    def match(i, best):
                        start = (end - 1 - i) * LANES
                        at = sub + (start + LANES)
                        for g in reversed(range(0, LANES, 8)):
                            tall = tall_v[pl.ds(pl.multiple_of(start + g, 8), 8), :]
                            at = at - 8
                            best = [jnp.where(tall == w, at, f) for w, f in zip(wide, best)]
                        return best
                    best = lax.fori_loop(0, end, match, [sub + n for _ in blocks])
                    for b, f in zip(blocks, best):
                        origin = jnp.where(blk == b, jnp.min(f, axis=0, keepdims=True), origin)
                owner = jnp.where(origin == here, x >> shift, N_DEV)
                count = running_count(jnp.concatenate([owner - o for o in range(N_DEV)], axis=0) == 0)
                rank = own_count = count[0:n_blk]
                for o in range(1, N_DEV):
                    part = count[o * n_blk:(o + 1) * n_blk]
                    rank = jnp.where(owner == o, part, rank)
                    own_count = jnp.where(me == o, part, own_count)
                list_v[...] = fetch_list(x, owner == me, own_count, range(early, n_blk))
                rest_cp.start()
                slot = source = (owner * n + blk * LANES + rank - 1) * wpr
                for b in range(n_blk):
                    there = jnp.take_along_axis(
                        jnp.broadcast_to(slot[b:b + 1], slot.shape), origin & (LANES - 1), axis=1)
                    source = jnp.where((origin >> 7) == b, there, source)
                source_v[...] = source
                count_v[...] = count
                for cp in plan_cps:
                    cp.start()
                rest_cp.wait()
            ship(early, fetch(early))
            stream(early + 1, n_blk, fetch(early + 1))
            for cp in plan_cps:
                cp.wait()

            def upto(o, b, lane):
                return count_s[o * n_blk + b, lane - 1] if lane else 0

            def total(o):
                return lax.fori_loop(0, n_blk, lambda b, t: t + upto(o, b, LANES), jnp.int32(0))

            t_me, t_right, t_far, t_left = total(me), total(right), total(far), total(left)

            def rightward(bias, seen):
                return jnp.clip((bias + seen) >> 1, 0, seen)

            def each_segment(step, carry):
                carry = lax.fori_loop(0, n_blk - 1, lambda b, c: step(b, b, 0, LANES, c), carry)
                for k, (lo, hi) in enumerate(zip((0,) + tail, tail + (LANES,))):
                    carry = step(n_blk - 1 + k, n_blk - 1, lo, hi, carry)

            def relay(s, b, lo, hi, seen):
                new = []
                for way, (src, bias) in enumerate(((left, t_far - t_me), (right, t_me - t_far))):
                    slot = src * n + b * LANES
                    if lo == 0:
                        whole = upto(src, b, LANES)

                        @pl.when(whole > 0)
                        def _():
                            hop(slot, whole, own_sem, b, way).wait_recv()
                    skip = upto(src, b, lo)
                    c = upto(src, b, hi) - skip
                    cut = rightward(bias, seen[way] + c) - rightward(bias, seen[way])
                    off, m = (0, cut) if way == 0 else (cut, c - cut)

                    @pl.when(m > 0)
                    def _():
                        hop(slot + skip + off, m, far_sem, s, way).start()
                    new.append(seen[way] + c)
                return tuple(new)
            each_segment(relay, (jnp.int32(0), jnp.int32(0)))

            sent = (t_me + rightward(t_far - t_me, t_left),
                    t_me + t_right - rightward(t_me - t_far, t_right))

            def place(s, b, lo, hi, seen):
                skip = upto(far, b, lo)
                c = upto(far, b, hi) - skip
                bias = t_right - t_left
                cut = rightward(bias, seen + c) - rightward(bias, seen)
                for way, (off, m) in enumerate(((0, cut), (cut, c - cut))):
                    @pl.when(m > 0)
                    def _():
                        hop(far * n + b * LANES + skip + off, m, far_sem, s, way).wait_recv()
                with scope("mv"):
                    for i in range(lo, hi):
                        tmp_v[pl.ds(i * wpr, wpr), :] = comm_v[pl.ds(source_s[b, i], wpr), :]
                    for i in range(lo, hi, 16):
                        at = pl.ds(pl.multiple_of(b * LANES + i, 16), 16)
                        for j in range(wpr):
                            ev = tmp_v[pl.ds(i * wpr + j, 8, stride=2 * wpr), :]
                            od = tmp_v[pl.ds((i + 1) * wpr + j, 8, stride=2 * wpr), :]
                            low = (ev & 0xFFFF) | (od << 16)
                            high = (ev >> 16) | (od & jnp.uint32(0xFFFF0000))
                            out_ref[at, pl.ds(2 * j * LANES, LANES)] = pltpu.bitcast(low, jnp.bfloat16)
                            out_ref[at, pl.ds((2 * j + 1) * LANES, LANES)] = pltpu.bitcast(high, jnp.bfloat16)
                return seen + c
            each_segment(place, jnp.int32(0))

            for way in range(2):
                @pl.when(sent[way] > 0)
                def _():
                    hop(0, sent[way], own_sem, 0, way).wait_send()

        i32 = jnp.int32
        return pl.pallas_call(
            body,
            out_shape=jax.ShapeDtypeStruct((n, d), jnp.bfloat16),
            in_specs=[pl.BlockSpec(memory_space=pl.ANY), pl.BlockSpec(memory_space=pl.ANY)],
            out_specs=pl.BlockSpec(memory_space=pltpu.VMEM),
            scratch_shapes=[
                pltpu.SMEM((1, LANES), i32),
                pltpu.SMEM((LANES,), i32),
                pltpu.SMEM((1, n), i32),
                pltpu.SMEM((N_DEV * n_blk, LANES), i32),
                pltpu.SMEM((n_blk, LANES), i32),
                pltpu.VMEM((n_blk, LANES), i32),
                pltpu.VMEM((1, n), i32),
                pltpu.VMEM((N_DEV * n_blk, LANES), i32),
                pltpu.VMEM((n_blk, LANES), i32),
                pltpu.VMEM((n, LANES), i32),
                pltpu.VMEM((n + GROUP * n_piece, 1, d), jnp.float32),
                pltpu.VMEM((N_DEV * n * wpr, LANES), jnp.uint32),
                pltpu.VMEM((LANES * wpr, LANES), jnp.uint32),
                pltpu.SemaphoreType.DMA((3,)),
                pltpu.SemaphoreType.DMA((n_blk + n_piece,)),
                pltpu.SemaphoreType.DMA((2,)),
                pltpu.SemaphoreType.DMA((2 * n_blk,)),
                pltpu.SemaphoreType.DMA((2 * n_seg,)),
                pltpu.SemaphoreType.REGULAR,
            ],
            compiler_params=pltpu.CompilerParams(
                collective_id=0, vmem_limit_bytes=64 << 20, flags=flags,
                disable_bounds_checks=not checks, disable_semaphore_checks=not checks),
            interpret=interpret,
        )(table, idx.reshape(n_blk, LANES))
    return kernel


def pallas_dist_embed_lookup_i_n2048_v16384_d1024_kernel(table, idx):
    return make()(table, idx)
```

```python
import jax
import jax.numpy as jnp
from jax import lax
from jax.experimental import pallas as pl
from jax.experimental.pallas import tpu as pltpu

N_DEV = 4
BLOCK = 128
GROUP = 8
N_PIECE = 5
EARLY_BLOCKS = 5
TAIL = (64, 96, 112)
RIGHT, LEFT = 0, 1


def _lookup_body(table_ref, idx_ref, out_ref,
                 head_s, pick_s, list_s, count_s, source_s,
                 idx_v, list_v, count_v, source_v, tall_v, rows_v, comm_v, order_v,
                 misc_sem, fetch_sem, send_sem, own_sem, far_sem, ready_sem):
    v_loc, d = table_ref.shape
    n_blk = idx_ref.shape[0]
    n = n_blk * BLOCK
    shift = v_loc.bit_length() - 1
    wpr = d // (2 * BLOCK)

    head_cp = pltpu.make_async_copy(idx_ref.at[pl.ds(0, 1)], head_s, misc_sem.at[0])
    idx_cp = pltpu.make_async_copy(idx_ref, idx_v, misc_sem.at[1])
    head_cp.start()
    idx_cp.start()

    me = lax.axis_index("i")
    right, far, left = (me + 1) & 3, (me + 2) & 3, (me + 3) & 3
    odd = (me & 1) == 1

    def notify(sem, chip):
        pl.semaphore_signal(sem, 1, device_id=(chip,), device_id_type=pl.DeviceIdType.MESH)

    barrier = pltpu.get_barrier_semaphore()

    @pl.when(odd)
    def _():
        notify(barrier, 2)
        pl.semaphore_wait(barrier, 1)
        notify(ready_sem, 0)

    @pl.when(me == 0)
    def _():
        notify(barrier, 1)
        notify(barrier, 3)

    @pl.when(me == 2)
    def _():
        pl.semaphore_wait(barrier, 2)
        notify(ready_sem, 1)
        notify(ready_sem, 3)

    down = lax.broadcasted_iota(jnp.int32, (BLOCK, BLOCK), 0)
    across = lax.broadcasted_iota(jnp.int32, (BLOCK, BLOCK), 1)

    def as_bits(flag):
        return jnp.where(flag, 1.0, 0.0).astype(jnp.bfloat16)

    def running_count(flag):
        return jnp.dot(as_bits(flag), as_bits(down <= across),
                       preferred_element_type=jnp.float32).astype(jnp.int32)

    def fetch_list(x, flag, count, blocks):
        half = (shift + 1) // 2
        local = x & (v_loc - 1)
        digits = jnp.concatenate([local >> half, local & ((1 << half) - 1)], axis=0)
        digits = digits.astype(jnp.float32).astype(jnp.bfloat16)
        goal = jnp.where(flag, count - 1, -1)
        blk = lax.broadcasted_iota(jnp.int32, x.shape, 0)
        front = jnp.zeros_like(x)
        for b in blocks:
            got = lax.dot_general(digits, as_bits(goal[b:b + 1] == down), (((1,), (1,)), ((), ())),
                                  preferred_element_type=jnp.float32).astype(jnp.int32)
            front = jnp.where(blk == b, (got[:x.shape[0]] << half) | got[x.shape[0]:], front)
        return (front | (count << shift)).reshape(1, x.shape[0] * BLOCK)

    def clear_rows(at, size):
        rows_v[pl.ds(at, size)] = jnp.zeros((size, 1, d), rows_v.dtype)

    def fetch_row(entry, at, sem):
        pltpu.make_async_copy(
            table_ref.at[pl.ds(entry & (v_loc - 1), 1)], rows_v.at[at], sem).start()

    def fetch(b, skip=0):
        c = (list_s[0, b * BLOCK + BLOCK - 1] >> shift) - skip
        clear_rows(b * BLOCK + jnp.minimum(c & -GROUP, BLOCK - GROUP), GROUP)
        lax.fori_loop(b * BLOCK, b * BLOCK + c,
                      lambda k, _: fetch_row(list_s[0, k + skip], k, fetch_sem.at[b]), None)
        return c

    def pack(base, c, sem, slot, one_group=False):
        @pl.when(c > 0)
        def _():
            got = rows_v.at[pl.ds(base, c)]
            pltpu.make_async_copy(got, got, sem).wait()

        def group(g, _):
            rows = rows_v[pl.ds(base + GROUP * g, GROUP)].reshape(2 * GROUP * wpr, BLOCK)
            comm_v[pl.ds((slot + GROUP * g) * wpr, GROUP * wpr), :] = pltpu.bitcast(
                rows.astype(jnp.bfloat16), jnp.uint32)
        if one_group:
            group(0, None)
        else:
            lax.fori_loop(0, (c + GROUP - 1) >> 3, group, None)

    def hop(slot, c, recv_sems, k, way):
        part = comm_v.at[pl.ds(slot * wpr, c * wpr)]
        return pltpu.make_async_remote_copy(
            part, part, send_sem.at[way], recv_sems.at[2 * k + way],
            device_id=((me + 1 + 2 * way) & 3,), device_id_type=pl.DeviceIdType.MESH)

    def send(slot, c, b, way):
        @pl.when(c > 0)
        def _():
            hop(slot, c, own_sem, b, way).start()

    def ship(b, c):
        slot = me * n + b * BLOCK
        pack(b * BLOCK, c, fetch_sem.at[b], slot)
        send(slot, c, b, RIGHT)
        send(slot, c, b, LEFT)

    def scan(lo, hi, others):
        for i in range(lo, hi):
            entry = head_s[0, i] ^ (me << shift)
            pick_s[i - others] = entry
            foreign = (entry & ((N_DEV - 1) << shift)).astype(jnp.uint32)
            others = others + jnp.minimum(foreign, jnp.uint32(1)).astype(jnp.int32)
        return others

    def fetch_piece(k, picked, fetched, room):
        c = jnp.minimum(picked - fetched, room)

        @pl.when(c > 0)
        def _():
            for j in range(room):
                @pl.when(j < c)
                def _():
                    fetch_row(pick_s[fetched + j], n + GROUP * k + j, fetch_sem.at[n_blk + k])
        return fetched + c

    def pack_piece(k, lo, hi):
        pack(n + GROUP * k, hi - lo, fetch_sem.at[n_blk + k], me * n + lo, one_group=True)

    near = jnp.where(me == 1, LEFT, RIGHT)

    def send_early(lo, hi):
        send(me * n + lo, hi - lo, 0, near)
        send(me * n + lo, jnp.where(odd, 0, hi - lo), 0, 1 - near)

    quick = pl.ds(0, EARLY_BLOCKS * BLOCK)
    quick_cp = pltpu.make_async_copy(list_v.at[:, quick], list_s.at[:, quick], misc_sem.at[2])
    clear_rows(n, GROUP * N_PIECE)

    head_cp.wait()
    others = scan(0, 16, jnp.int32(0))
    end0 = fetch_piece(0, 16 - others, jnp.int32(0), 4)
    idx_cp.wait()
    x = idx_v[...]
    mine = ((x >> shift) & (N_DEV - 1)) == me
    count = running_count(mine)
    others = scan(16, 44, others)
    end1 = fetch_piece(1, 44 - others, end0, 6)
    others = scan(44, 100, others)
    list_v[:, 0:8 * BLOCK] = fetch_list(x[0:8], mine[0:8], count[0:8], range(EARLY_BLOCKS))
    quick_cp.start()
    end2 = fetch_piece(2, 100 - others, end1, 5)
    pack_piece(0, 0, end0)

    @pl.when(me == 0)
    def _():
        pl.semaphore_wait(ready_sem, 2)
    send_early(0, end0)
    end3 = fetch_piece(3, 100 - others, end2, 8)
    pack_piece(1, end0, end1)
    send_early(end0, end1)
    others = scan(100, 120, others)
    end4 = fetch_piece(4, 120 - others, end3, 6)
    pack_piece(2, end1, end2)
    send_early(end1, end2)
    quick_cp.wait()
    c_rest = fetch(0, skip=end4)
    pack_piece(3, end2, end3)
    send_early(end2, end3)
    c_second = fetch(1)
    pack_piece(4, end3, end4)
    send(me * n + end3, end4 - end3, 0, near)

    @pl.when(odd)
    def _():
        pl.semaphore_wait(ready_sem, 1)
    unsent = jnp.where(odd, 0, end3)
    send(me * n + unsent, end4 - unsent, 0, 1 - near)
    pack(0, c_rest, fetch_sem.at[0], me * n + end4)
    send(me * n + end4, c_rest, 0, near)
    send(me * n + end4, c_rest, 0, 1 - near)
    ship(1, c_second)
    c_last = fetch(2)
    for b in range(2, EARLY_BLOCKS - 1):
        c_now, c_last = c_last, fetch(b + 1)
        ship(b, c_now)

    x = idx_v[...] & (N_DEV * v_loc - 1)
    blk = lax.broadcasted_iota(jnp.int32, (n_blk, BLOCK), 0)
    here = blk * BLOCK + lax.broadcasted_iota(jnp.int32, (n_blk, BLOCK), 1)
    for b in range(n_blk):
        tall_v[pl.ds(b * BLOCK, BLOCK), :] = jnp.broadcast_to(x[b:b + 1], (BLOCK, BLOCK)).T
    ship(EARLY_BLOCKS - 1, c_last)
    sub = lax.broadcasted_iota(jnp.int32, (8, BLOCK), 0)
    origin = here
    for end in range(n_blk, EARLY_BLOCKS, -4):
        blocks = range(max(end - 4, EARLY_BLOCKS), end)
        wide = [jnp.broadcast_to(x[b:b + 1], (8, BLOCK)) for b in blocks]

        def match(i, found):
            start = pl.multiple_of((end - 1 - i) * BLOCK, BLOCK)
            tall = tall_v[pl.ds(start, BLOCK), :]
            at = sub + (start + BLOCK)
            for g in reversed(range(0, BLOCK, 8)):
                at = at - 8
                found = [jnp.where(tall[g:g + 8] == w, at, f) for w, f in zip(wide, found)]
            return found
        found = lax.fori_loop(0, end, match, [sub + n for _ in blocks])
        for b, f in zip(blocks, found):
            origin = jnp.where(blk == b, jnp.min(f, axis=0, keepdims=True), origin)

    sender = jnp.where(origin == here, x >> shift, N_DEV)
    count = running_count(jnp.concatenate([sender - o for o in range(N_DEV)], axis=0) == 0)
    rank = my_count = count[0:n_blk]
    for o in range(1, N_DEV):
        part = count[o * n_blk:(o + 1) * n_blk]
        rank = jnp.where(sender == o, part, rank)
        my_count = jnp.where(me == o, part, my_count)

    rest = pl.ds(EARLY_BLOCKS * BLOCK, n - EARLY_BLOCKS * BLOCK)
    rest_cp = pltpu.make_async_copy(list_v.at[:, rest], list_s.at[:, rest], misc_sem.at[0])
    count_cp = pltpu.make_async_copy(count_v, count_s, misc_sem.at[1])
    source_cp = pltpu.make_async_copy(source_v, source_s, misc_sem.at[2])
    list_v[...] = fetch_list(x, sender == me, my_count, range(EARLY_BLOCKS, n_blk))
    rest_cp.start()
    landing = source = (sender * n + blk * BLOCK + rank - 1) * wpr
    for b in range(n_blk):
        there = jnp.take_along_axis(
            jnp.broadcast_to(landing[b:b + 1], landing.shape), origin & (BLOCK - 1), axis=1)
        source = jnp.where((origin & -BLOCK) == b * BLOCK, there, source)
    source_v[...] = source
    count_v[...] = count
    count_cp.start()
    source_cp.start()
    rest_cp.wait()
    ship(EARLY_BLOCKS, fetch(EARLY_BLOCKS))

    def fetch_and_ship(b, c):
        c_next = lax.cond(b + 1 < n_blk, lambda: fetch(b + 1), lambda: jnp.int32(0))
        ship(b, c)
        return c_next
    lax.fori_loop(EARLY_BLOCKS + 1, n_blk, fetch_and_ship, fetch(EARLY_BLOCKS + 1))
    count_cp.wait()
    source_cp.wait()

    def sent_for(o, b, positions):
        return count_s[o * n_blk + b, positions - 1] if positions else 0

    def total(o):
        return lax.fori_loop(0, n_blk, lambda b, t: t + sent_for(o, b, BLOCK), jnp.int32(0))

    t_me, t_right, t_far, t_left = total(me), total(right), total(far), total(left)

    def rightward(bias, seen):
        return jnp.clip((bias + seen) >> 1, 0, seen)

    def split(o, b, lo, hi, bias, seen):
        skip = sent_for(o, b, lo)
        c = sent_for(o, b, hi) - skip
        cut = rightward(bias, seen + c) - rightward(bias, seen)
        slot = o * n + b * BLOCK + skip
        return c, ((slot, cut), (slot + cut, c - cut))

    def each_segment(step, carry):
        carry = lax.fori_loop(0, n_blk - 1, lambda b, c: step(b, b, 0, BLOCK, c), carry)
        for k, (lo, hi) in enumerate(zip((0,) + TAIL, TAIL + (BLOCK,))):
            carry = step(n_blk - 1 + k, n_blk - 1, lo, hi, carry)

    def relay(s, b, lo, hi, seen):
        now_seen = []
        for way, o, bias in ((RIGHT, left, t_far - t_me), (LEFT, right, t_me - t_far)):
            if lo == 0:
                whole = sent_for(o, b, BLOCK)

                @pl.when(whole > 0)
                def _():
                    hop(o * n + b * BLOCK, whole, own_sem, b, way).wait_recv()
            c, parts = split(o, b, lo, hi, bias, seen[way])
            slot, m = parts[way]

            @pl.when(m > 0)
            def _():
                hop(slot, m, far_sem, s, way).start()
            now_seen.append(seen[way] + c)
        return tuple(now_seen)
    each_segment(relay, (jnp.int32(0), jnp.int32(0)))
    sent = (t_me + rightward(t_far - t_me, t_left),
            t_me + t_right - rightward(t_me - t_far, t_right))

    def place(s, b, lo, hi, seen):
        c, parts = split(far, b, lo, hi, t_right - t_left, seen)
        for way, (slot, m) in enumerate(parts):
            @pl.when(m > 0)
            def _():
                hop(slot, m, far_sem, s, way).wait_recv()
        for i in range(lo, hi):
            order_v[pl.ds(i * wpr, wpr), :] = comm_v[pl.ds(source_s[b, i], wpr), :]
        at = pl.ds(pl.multiple_of(b * BLOCK + lo, 16), hi - lo)
        for j in range(wpr):
            upper = order_v[pl.ds(lo * wpr + j, (hi - lo) // 2, stride=2 * wpr), :]
            lower = order_v[pl.ds((lo + 1) * wpr + j, (hi - lo) // 2, stride=2 * wpr), :]
            out_ref[at, pl.ds(2 * j * BLOCK, BLOCK)] = pltpu.bitcast(
                (upper & 0xFFFF) | (lower << 16), jnp.bfloat16)
            out_ref[at, pl.ds((2 * j + 1) * BLOCK, BLOCK)] = pltpu.bitcast(
                (upper >> 16) | (lower & jnp.uint32(0xFFFF0000)), jnp.bfloat16)
        return seen + c
    each_segment(place, jnp.int32(0))

    for way in (RIGHT, LEFT):
        @pl.when(sent[way] > 0)
        def _():
            hop(0, sent[way], own_sem, 0, way).wait_send()


def pallas_dist_embed_lookup_i_n2048_v16384_d1024_kernel(table: jax.Array, idx: jax.Array):
    (n,), (_, d) = idx.shape, table.shape
    n_blk, wpr = n // BLOCK, d // (2 * BLOCK)
    i32 = jnp.int32
    return pl.pallas_call(
        _lookup_body,
        out_shape=jax.ShapeDtypeStruct((n, d), jnp.bfloat16),
        in_specs=[pl.BlockSpec(memory_space=pl.ANY), pl.BlockSpec(memory_space=pl.ANY)],
        out_specs=pl.BlockSpec(memory_space=pltpu.VMEM),
        scratch_shapes=[
            pltpu.SMEM((1, BLOCK), i32),
            pltpu.SMEM((BLOCK,), i32),
            pltpu.SMEM((1, n), i32),
            pltpu.SMEM((N_DEV * n_blk, BLOCK), i32),
            pltpu.SMEM((n_blk, BLOCK), i32),
            pltpu.VMEM((n_blk, BLOCK), i32),
            pltpu.VMEM((1, n), i32),
            pltpu.VMEM((N_DEV * n_blk, BLOCK), i32),
            pltpu.VMEM((n_blk, BLOCK), i32),
            pltpu.VMEM((n, BLOCK), i32),
            pltpu.VMEM((n + GROUP * N_PIECE, 1, d), table.dtype),
            pltpu.VMEM((N_DEV * n * wpr, BLOCK), jnp.uint32),
            pltpu.VMEM((BLOCK * wpr, BLOCK), jnp.uint32),
            pltpu.SemaphoreType.DMA((3,)),
            pltpu.SemaphoreType.DMA((n_blk + N_PIECE,)),
            pltpu.SemaphoreType.DMA((2,)),
            pltpu.SemaphoreType.DMA((2 * n_blk,)),
            pltpu.SemaphoreType.DMA((2 * (n_blk + len(TAIL)),)),
            pltpu.SemaphoreType.REGULAR,
        ],
        compiler_params=pltpu.CompilerParams(
            collective_id=0,
            vmem_limit_bytes=64 << 20,
            disable_bounds_checks=True,
            disable_semaphore_checks=True,
        ),
    )(table, idx.reshape(n_blk, BLOCK))
```
